```python
import numpy as np

kernel_name = "dist_mean_ax0_xy_m1024_n512"

def setup_inputs():
    return {"x": np.random.randn(2048, 1024).astype(np.float32)}

def reference(x: np.ndarray) -> np.ndarray:
    return np.mean(x, axis=0, keepdims=True)
```

```python
import jax
import jax.numpy as jnp
from jax import lax
from jax.experimental import pallas as pl
from jax.experimental.pallas import tpu as pltpu

N_CHUNKS = 8


def pallas_dist_mean_ax0_xy_m1024_n512_kernel(x: jax.Array):
    m, n = x.shape
    rows = m // N_CHUNKS
    inv_total = 1.0 / (2 * m)

    def body(x_hbm, out_ref, buf, send_buf, recv_buf, load_sems, send_sem, recv_sem):
        my_x = lax.axis_index("x")
        my_y = lax.axis_index("y")
        peer = (1 - my_x, my_y)

        copies = []
        for c in range(N_CHUNKS):
            cp = pltpu.make_async_copy(
                x_hbm.at[pl.ds(c * rows, rows)],
                buf.at[pl.ds(c * rows, rows)],
                load_sems.at[c],
            )
            cp.start()
            copies.append(cp)

        barrier = pltpu.get_barrier_semaphore()
        pl.semaphore_signal(
            barrier, inc=1, device_id=peer, device_id_type=pl.DeviceIdType.MESH
        )

        acc = jnp.zeros((8, n), jnp.float32)
        for c in range(N_CHUNKS):
            copies[c].wait()
            chunk = buf[pl.ds(c * rows, rows), :]
            acc = acc + jnp.sum(chunk.reshape(rows // 8, 8, n), axis=0)
        send_buf[...] = jnp.sum(acc, axis=0, keepdims=True)

        pl.semaphore_wait(barrier, 1)
        rdma = pltpu.make_async_remote_copy(
            src_ref=send_buf,
            dst_ref=recv_buf,
            send_sem=send_sem,
            recv_sem=recv_sem,
            device_id=peer,
            device_id_type=pl.DeviceIdType.MESH,
        )
        rdma.start()
        rdma.wait()
        out_ref[...] = (send_buf[...] + recv_buf[...]) * inv_total

    return pl.pallas_call(
        body,
        out_shape=jax.ShapeDtypeStruct((1, n), jnp.float32),
        in_specs=[pl.BlockSpec(memory_space=pl.ANY)],
        out_specs=pl.BlockSpec(memory_space=pltpu.VMEM),
        scratch_shapes=[
            pltpu.VMEM((m, n), jnp.float32),
            pltpu.VMEM((1, n), jnp.float32),
            pltpu.VMEM((1, n), jnp.float32),
            pltpu.SemaphoreType.DMA((N_CHUNKS,)),
            pltpu.SemaphoreType.DMA,
            pltpu.SemaphoreType.DMA,
        ],
        compiler_params=pltpu.CompilerParams(collective_id=0),
    )(x)
```

```python
import jax
import jax.numpy as jnp
from jax import lax
from jax.experimental import pallas as pl
from jax.experimental.pallas import tpu as pltpu

CHUNKS = (512, 256, 128, 64, 32, 16, 8, 8)


def pallas_dist_mean_ax0_xy_m1024_n512_kernel(x: jax.Array):
    m, n = x.shape
    assert sum(CHUNKS) == m
    inv_total = 1.0 / (2 * m)
    starts = [sum(CHUNKS[:i]) for i in range(len(CHUNKS))]

    def body(x_hbm, out_ref, buf, send_buf, recv_buf, load_sems, send_sem, recv_sem):
        my_x = lax.axis_index("x")
        my_y = lax.axis_index("y")
        peer = (1 - my_x, my_y)

        copies = []
        for c, (s, r) in enumerate(zip(starts, CHUNKS)):
            cp = pltpu.make_async_copy(
                x_hbm.at[pl.ds(s, r)],
                buf.at[pl.ds(s, r)],
                load_sems.at[c],
            )
            cp.start()
            copies.append(cp)

        barrier = pltpu.get_barrier_semaphore()
        pl.semaphore_signal(
            barrier, inc=1, device_id=peer, device_id_type=pl.DeviceIdType.MESH
        )

        acc = jnp.zeros((8, n), jnp.float32)
        for c, (s, r) in enumerate(zip(starts, CHUNKS)):
            copies[c].wait()
            chunk = buf[pl.ds(s, r), :]
            acc = acc + jnp.sum(chunk.reshape(r // 8, 8, n), axis=0)
        send_buf[...] = jnp.sum(acc, axis=0, keepdims=True)

        pl.semaphore_wait(barrier, 1)
        rdma = pltpu.make_async_remote_copy(
            src_ref=send_buf,
            dst_ref=recv_buf,
            send_sem=send_sem,
            recv_sem=recv_sem,
            device_id=peer,
            device_id_type=pl.DeviceIdType.MESH,
        )
        rdma.start()
        rdma.wait()
        out_ref[...] = (send_buf[...] + recv_buf[...]) * inv_total

    return pl.pallas_call(
        body,
        out_shape=jax.ShapeDtypeStruct((1, n), jnp.float32),
        in_specs=[pl.BlockSpec(memory_space=pl.ANY)],
        out_specs=pl.BlockSpec(memory_space=pltpu.VMEM),
        scratch_shapes=[
            pltpu.VMEM((m, n), jnp.float32),
            pltpu.VMEM((1, n), jnp.float32),
            pltpu.VMEM((1, n), jnp.float32),
            pltpu.SemaphoreType.DMA((len(CHUNKS),)),
            pltpu.SemaphoreType.DMA,
            pltpu.SemaphoreType.DMA,
        ],
        compiler_params=pltpu.CompilerParams(collective_id=0),
    )(x)
```
